```python
import numpy as np

kernel_name = "dist_sparse_attn_blocksparse_qseq_b2_sq256_skv256_hq4_dh64"

def setup_inputs():
    x = np.random.randn(2, 1024, 512).astype(np.float32)
    Wq = np.random.randn(512, 1024).astype(np.float32) * 0.02
    K_ext = np.random.randn(2, 256, 16, 64).astype(np.float32)
    V_ext = np.random.randn(2, 256, 16, 64).astype(np.float32)
    Wo = np.random.randn(1024, 512).astype(np.float32) * 0.02
    return {"x": x, "Wq": Wq, "K_ext": K_ext, "V_ext": V_ext, "Wo": Wo}

def reference(x, Wq, K_ext, V_ext, Wo):
    B, Sq, Skv, Hq, Dh = 2, 1024, 256, 16, 64
    Q = (x @ Wq).reshape(B, Sq, Hq, Dh)
    qb = (np.arange(Sq) // 64)[:, None]
    kb = (np.arange(Skv) // 64)[None, :]
    mask = (qb == kb) | (kb == 0) | ((qb + kb) % 3 == 0)
    scores = np.einsum('bihd,bjhd->bhij', Q, K_ext).astype(np.float32) * 0.125
    scores = np.where(mask[None, None, :, :], scores, -1e9)
    scores_max = scores.max(axis=-1, keepdims=True)
    w = np.exp(scores - scores_max)
    row_keep = mask.any(axis=1)
    w_sum = np.where(row_keep[None, None, :, None], w.sum(axis=-1, keepdims=True), 1.0)
    w = w / w_sum
    w = np.where(row_keep[None, None, :, None], w, 0.0)
    ctx = np.einsum('bhij,bjhd->bihd', w, V_ext).reshape(B, Sq, Hq * Dh)
    return ctx @ Wo
```

```python
import jax
import jax.numpy as jnp
from jax import lax
from jax.experimental import pallas as pl
from jax.experimental.pallas import tpu as pltpu

N_DEV = 4
B = 2
SQ = 256
SKV = 256
DM = 512
DH = 64
BLK = 64
ROWS = B * SQ
NEG = -1e9
BF = jnp.bfloat16
F32 = jnp.float32

SLOT_OFF = (0, 3, 1, 2)


def _kernel(x_hbm, wq_hbm, kt_hbm, vt_hbm, wo_hbm, out_ref,
            xf, xb, wqf, wof, wq_all, wo_all, ktf, vtf, ctx,
            lsem, ssem, rsem):
    me = lax.axis_index("i")
    left = (me + 3) % N_DEV
    right = (me + 1) % N_DEV

    bar = pltpu.get_barrier_semaphore()
    for nbr in (left, right):
        pl.semaphore_signal(bar, inc=1, device_id=(nbr,),
                            device_id_type=pl.DeviceIdType.MESH)

    cp_wq = pltpu.make_async_copy(wq_hbm, wqf, lsem.at[0])
    cp_wq.start()
    cp_x = pltpu.make_async_copy(x_hbm, xf, lsem.at[1])
    cp_x.start()
    cp_kv = []
    for s in range(4):
        grp = (me + SLOT_OFF[s]) % N_DEV
        ck = pltpu.make_async_copy(kt_hbm.at[:, pl.ds(2 * grp, 2)], ktf.at[s],
                                   lsem.at[3 + 2 * s])
        cv = pltpu.make_async_copy(vt_hbm.at[:, pl.ds(2 * grp, 2)], vtf.at[s],
                                   lsem.at[4 + 2 * s])
        ck.start()
        cv.start()
        cp_kv.append((ck, cv))
        if s == 0:
            cp_wo = pltpu.make_async_copy(wo_hbm, wof, lsem.at[2])
            cp_wo.start()

    sends = []

    def rcopy(src, dst, ridx, tgt):
        return pltpu.make_async_remote_copy(
            src, dst, ssem.at[0], rsem.at[ridx],
            device_id=(tgt,), device_id_type=pl.DeviceIdType.MESH)

    def send(src, dst, ridx, tgt):
        c = rcopy(src, dst, ridx, tgt)
        c.start()
        sends.append(c)

    def recv_wait(dst, ridx):
        rcopy(dst, dst, ridx, me).wait_recv()

    def rq(slot, h):
        return (slot - 1) * 2 + h

    def ro(slot, h):
        return 6 + (slot - 1) * 2 + h

    def rod(h, c):
        return 10 + h * 4 + c

    cp_wq.wait()
    for h in range(2):
        wq_all[0, h] = wqf[:, h * 128:(h + 1) * 128].astype(BF)

    pl.semaphore_wait(bar, 2)

    send(wq_all.at[0, 0], wq_all.at[1, 0], rq(1, 0), right)
    send(wq_all.at[0, 1], wq_all.at[2, 1], rq(2, 1), left)
    send(wq_all.at[0, 1], wq_all.at[1, 1], rq(1, 1), right)
    send(wq_all.at[0, 0], wq_all.at[2, 0], rq(2, 0), left)

    cp_wo.wait()
    for h in range(2):
        for c in range(4):
            wo_all[0, h, c] = wof[h * 128:(h + 1) * 128,
                                  c * 128:(c + 1) * 128].astype(BF)

    cp_x.wait()
    for b in range(B):
        xb[b * SQ:(b + 1) * SQ, :] = xf[b].astype(BF)

    row = lax.broadcasted_iota(jnp.int32, (SQ, SKV), 0)
    col = lax.broadcasted_iota(jnp.int32, (SQ, SKV), 1)
    qb = me * (SQ // BLK) + row // BLK
    kb = col // BLK
    mask = (qb == kb) | (kb == 0) | (lax.rem(qb + kb, 3) == 0)
    lane = lax.broadcasted_iota(jnp.int32, (SQ, 128), 1)
    lo = lane < DH

    def attend(slot, h):
        q = jnp.dot(xb[...], wq_all[slot, h], preferred_element_type=F32)
        q = (q * 0.125).astype(BF)
        zero = jnp.zeros((SQ, 128), BF)
        for b in range(B):
            qb_ = q[b * SQ:(b + 1) * SQ]
            kt = ktf[slot, b, h].astype(BF)
            vt = vtf[slot, b, h].astype(BF)
            res = []
            for sel in (lo, jnp.logical_not(lo)):
                qh = jnp.where(sel, qb_, zero)
                s = jnp.dot(qh, kt, preferred_element_type=F32)
                s = jnp.where(mask, s, NEG)
                m = jnp.max(s, axis=-1, keepdims=True)
                p = jnp.exp(s - m)
                l = jnp.sum(p, axis=-1, keepdims=True)
                r = lax.dot_general(p.astype(BF), vt, (((1,), (1,)), ((), ())),
                                    preferred_element_type=F32)
                res.append(r / l)
            cpair = jnp.where(lo, res[0], res[1])
            col0 = slot * 256 + h * 128
            ctx[b * SQ:(b + 1) * SQ, col0:col0 + 128] = cpair.astype(BF)

    def outproj(parts, cols, first):
        for c in cols:
            acc = None
            for (slot, h) in parts:
                col0 = slot * 256 + h * 128
                t = jnp.dot(ctx[:, col0:col0 + 128], wo_all[slot, h, c],
                            preferred_element_type=F32)
                acc = t if acc is None else acc + t
            for b in range(B):
                piece = acc[b * SQ:(b + 1) * SQ]
                if first:
                    out_ref[b, :, c * 128:(c + 1) * 128] = piece
                else:
                    out_ref[b, :, c * 128:(c + 1) * 128] += piece

    cp_kv[0][0].wait()
    cp_kv[0][1].wait()
    attend(0, 0)
    attend(0, 1)

    recv_wait(wq_all.at[1, 0], rq(1, 0))
    send(wq_all.at[1, 0], wq_all.at[3, 0], rq(3, 0), right)
    send(wo_all.at[0, 0], wo_all.at[1, 0], ro(1, 0), right)
    send(wo_all.at[0, 1], wo_all.at[1, 1], ro(1, 1), right)
    recv_wait(wq_all.at[2, 1], rq(2, 1))
    send(wq_all.at[2, 1], wq_all.at[3, 1], rq(3, 1), left)
    send(wo_all.at[0, 1], wo_all.at[2, 1], ro(2, 1), left)
    send(wo_all.at[0, 0], wo_all.at[2, 0], ro(2, 0), left)

    for s in (1, 2):
        cp_kv[s][0].wait()
        cp_kv[s][1].wait()
    attend(1, 0)
    attend(2, 1)

    recv_wait(wq_all.at[1, 1], rq(1, 1))
    attend(1, 1)
    recv_wait(wq_all.at[2, 0], rq(2, 0))
    attend(2, 0)

    outproj([(0, 0), (0, 1)], range(4), True)

    cp_kv[3][0].wait()
    cp_kv[3][1].wait()
    recv_wait(wq_all.at[3, 0], rq(3, 0))
    attend(3, 0)
    recv_wait(wq_all.at[3, 1], rq(3, 1))
    attend(3, 1)

    recv_wait(wo_all.at[1, 0], ro(1, 0))
    for c in range(4):
        send(wo_all.at[1, 0, c], wo_all.at[3, 0, c], rod(0, c), right)
    recv_wait(wo_all.at[2, 1], ro(2, 1))
    for c in range(4):
        send(wo_all.at[2, 1, c], wo_all.at[3, 1, c], rod(1, c), left)
    outproj([(1, 0), (2, 1)], range(4), False)

    recv_wait(wo_all.at[1, 1], ro(1, 1))
    recv_wait(wo_all.at[2, 0], ro(2, 0))
    outproj([(1, 1), (2, 0)], range(4), False)

    for c in range(4):
        recv_wait(wo_all.at[3, 0, c], rod(0, c))
        recv_wait(wo_all.at[3, 1, c], rod(1, c))
        outproj([(3, 0), (3, 1)], [c], False)

    for s in sends:
        s.wait_send()


def pallas_dist_sparse_attn_blocksparse_qseq_b2_sq256_skv256_hq4_dh64_kernel(
    x: jax.Array,
    Wq: jax.Array,
    K_ext: jax.Array,
    V_ext: jax.Array,
    Wo: jax.Array,
):
    kt = jnp.transpose(K_ext, (0, 2, 3, 1)).reshape(B, 8, 128, SKV)
    vt = jnp.transpose(V_ext, (0, 2, 3, 1)).reshape(B, 8, 128, SKV)

    hbm = pl.BlockSpec(memory_space=pltpu.HBM)
    return pl.pallas_call(
        _kernel,
        out_shape=jax.ShapeDtypeStruct((B, SQ, DM), F32),
        in_specs=[hbm] * 5,
        out_specs=pl.BlockSpec(memory_space=pltpu.VMEM),
        scratch_shapes=[
            pltpu.VMEM((B, SQ, DM), F32),
            pltpu.VMEM((ROWS, DM), BF),
            pltpu.VMEM((DM, 256), F32),
            pltpu.VMEM((256, DM), F32),
            pltpu.VMEM((4, 2, DM, 128), BF),
            pltpu.VMEM((4, 2, 4, 128, 128), BF),
            pltpu.VMEM((4, B, 2, 128, SKV), F32),
            pltpu.VMEM((4, B, 2, 128, SKV), F32),
            pltpu.VMEM((ROWS, 1024), BF),
            pltpu.SemaphoreType.DMA((11,)),
            pltpu.SemaphoreType.DMA((1,)),
            pltpu.SemaphoreType.DMA((18,)),
        ],
        compiler_params=pltpu.CompilerParams(
            collective_id=0,
            vmem_limit_bytes=64 * 1024 * 1024,
            disable_semaphore_checks=True,
        ),
    )(x, Wq, kt, vt, Wo)
```

```python
import contextlib
import jax
import jax.numpy as jnp
from jax import lax
from jax.experimental import pallas as pl
from jax.experimental.pallas import tpu as pltpu

SCOPES = False
def sc(n):
    return jax.named_scope(n) if SCOPES else contextlib.nullcontext()

N_DEV = 4
B = 2
SQ = 256
SKV = 256
DM = 512
DH = 64
BLK = 64
ROWS = B * SQ
NEG = -1e9
BF = jnp.bfloat16
F32 = jnp.float32
NT = (((1,), (1,)), ((), ()))
MESH = pl.DeviceIdType.MESH

SLOT_OFF = (0, 3, 1, 2)
WQ_PIECES = ((0, 16), (16, 48), (64, 64), (128, 128), (256, 256))
NF = 32
PAIR_ORDER = ((0, 0), (0, 1), (1, 0), (2, 1), (1, 1), (2, 0), (3, 0), (3, 1))
WO_FWD = ((0, 2), (2, 2), (4, 2), (6, 1), (7, 1))


def wo_loc(h, c, a):
    if c < 3:
        return h, 2 * c + a
    return a, 6 + h


def _kernel(x_hbm, wq_hbm, kt_hbm, vt_hbm, wo_hbm, out_ref,
            xf, xb, wqf, wof, wq_all, wo_all, ktf, vtf, ctx, wqs,
            lsem, ssem, rsem, ready):
    me = lax.axis_index("i")
    left = (me + 3) % N_DEV
    right = (me + 1) % N_DEV

    cp_wq = []
    for i, (r0, n) in enumerate(WQ_PIECES):
        c = pltpu.make_async_copy(wq_hbm.at[pl.ds(r0, n)], wqf.at[pl.ds(r0, n)],
                                  lsem.at[i])
        cp_wq.append(c)
    cp_wq[0].start()

    bar = pltpu.get_barrier_semaphore()
    odd = lax.rem(me, 2) == 1

    @pl.when(me != 2)
    def _():
        for nbr in (left, right):
            pl.semaphore_signal(bar, inc=1, device_id=(nbr,), device_id_type=MESH)

    @pl.when(me == 2)
    def _():
        pl.semaphore_wait(bar, 2)
        for nbr in (left, right):
            pl.semaphore_signal(ready, inc=1, device_id=(nbr,), device_id_type=MESH)

    sends = []

    def rcopy(src, dst, ridx, tgt):
        return pltpu.make_async_remote_copy(
            src, dst, ssem.at[0], rsem.at[ridx],
            device_id=(tgt,), device_id_type=MESH)

    def send(src, dst, ridx, tgt):
        c = rcopy(src, dst, ridx, tgt)
        c.start()
        sends.append(c)

    def recv_wait(dst, ridx):
        with sc(f"w{ridx}"):
            rcopy(dst, dst, ridx, me).wait_recv()

    def rq(slot, h):
        return (slot - 1) * 2 + h

    def ro(slot, half):
        return 6 + (slot - 1) * 2 + half

    def rod(half, k):
        return 10 + half * 5 + k

    fr = rcopy(wq_hbm.at[pl.ds(0, NF), pl.ds(128, 128)], wqs.at[0], 20, right)
    fl = rcopy(wq_hbm.at[pl.ds(0, NF), pl.ds(0, 128)], wqs.at[1], 21, left)

    @pl.when(odd)
    def _():
        pl.semaphore_wait(bar, 1)

    pl.when(me >= 2)(fr.start)
    pl.when((me == 1) | (me == 2))(fl.start)
    gr = rcopy(wqf.at[pl.ds(0, NF), pl.ds(128, 128)], wqs.at[0], 20, right)
    gl = rcopy(wqf.at[pl.ds(0, NF), pl.ds(0, 128)], wqs.at[1], 21, left)

    for c in cp_wq[1:]:
        c.start()
    cp_wo = pltpu.make_async_copy(wo_hbm, wof, lsem.at[7])
    cp_wo.start()
    cp_x = []
    for b in range(B):
        c = pltpu.make_async_copy(x_hbm.at[b], xf.at[b], lsem.at[5 + b])
        c.start()
        cp_x.append(c)
    cp_kv = {}
    for i, (s, h) in enumerate(PAIR_ORDER):
        pr = 2 * ((me + SLOT_OFF[s]) % N_DEV) + h
        ck = pltpu.make_async_copy(kt_hbm.at[:, pr], ktf.at[s, h],
                                   lsem.at[8 + 2 * i])
        cv = pltpu.make_async_copy(vt_hbm.at[:, pr], vtf.at[s, h],
                                   lsem.at[9 + 2 * i])
        ck.start()
        cv.start()
        cp_kv[(s, h)] = (ck, cv)


    to_r, to_l = [], []
    for i, (r0, n) in enumerate(WQ_PIECES):
        with sc("lwq"):
            cp_wq[i].wait()
        for h in range(2):
            wq_all[0, h, r0:r0 + n, :] = (
                wqf[r0:r0 + n, h * 128:(h + 1) * 128].astype(BF))
        if i == 0:
            with sc("bar"):
                @pl.when(me == 0)
                def _():
                    pl.semaphore_wait(bar, 2)
        rows = pl.ds(r0, n)
        cr = rcopy(wq_all.at[0, 0, rows], wq_all.at[1, 0, rows], rq(1, 0), right)
        cl = rcopy(wq_all.at[0, 1, rows], wq_all.at[2, 1, rows], rq(2, 1), left)
        to_r.append(cr)
        to_l.append(cl)
        pl.when(me != 1)(cr.start)
        pl.when(me != 3)(cl.start)
    sends += to_r + to_l + [gr, gl]

    with sc("rdy"):
        @pl.when(odd)
        def _():
            pl.semaphore_wait(ready, 1)

    @pl.when(me == 1)
    def _():
        for c in to_r:
            c.start()

    @pl.when(me == 3)
    def _():
        for c in to_l:
            c.start()

    pl.when(me < 2)(gr.start)
    pl.when((me == 0) | (me == 3))(gl.start)
    rest = pl.ds(NF, DM - NF)
    send(wq_all.at[0, 1, rest], wq_all.at[1, 1, rest], rq(1, 1), right)
    send(wq_all.at[0, 0, rest], wq_all.at[2, 0, rest], rq(2, 0), left)

    with sc("lwo"):
        cp_wo.wait()
    for h in range(2):
        for c in range(4):
            for a in range(2):
                hf, k = wo_loc(h, c, a)
                r0 = h * 128 + a * DH
                wo_all[0, hf, k] = wof[r0:r0 + DH, c * 128:(c + 1) * 128].astype(BF)
    send(wo_all.at[0, 0], wo_all.at[1, 0], ro(1, 0), right)
    send(wo_all.at[0, 1], wo_all.at[2, 1], ro(2, 1), left)

    for b in range(B):
        with sc("lx"):
            cp_x[b].wait()
        xb[b * SQ:(b + 1) * SQ, :] = xf[b].astype(BF)

    row = lax.broadcasted_iota(jnp.int32, (2 * BLK, SKV), 0)
    col = lax.broadcasted_iota(jnp.int32, (2 * BLK, SKV), 1)
    qb = me * (SQ // BLK) + 1 + row // BLK
    kb = col // BLK
    mask_mid = (qb == kb) | (kb == 0) | (lax.rem(qb + kb, 3) == 0)
    xk = 3 - lax.rem(me, 3)
    col1 = lax.broadcasted_iota(jnp.int32, (16, SKV), 1) // BLK
    off_ind = jnp.where((col1 == 0) | (col1 == xk), 0.0, 1.0).astype(BF)
    lo128 = lax.broadcasted_iota(jnp.int32, (128, 128), 1) < DH

    def gather_keys(t):
        t01 = t[:, :128]
        t23 = t[:, 128:]
        y = jnp.where(xk == 2, pltpu.roll(t23, 64, 1), t23)
        y = jnp.where(xk == 1, t01, y)
        return jnp.where(lo128, t01, y)

    hi128 = jnp.logical_not(lo128)
    zero = jnp.zeros((128, 128), BF)
    ones_m = jnp.ones((DH, SKV), BF)
    ones_o = jnp.ones((DH, 128), BF)

    def scores(slot, h):
        q = jnp.dot(xb[...], wq_all[slot, h], preferred_element_type=F32)
        q = (q * 0.125).astype(BF)
        out = []
        for b in range(B):
            ktf32 = ktf[slot, h, b]
            kt = ktf32.astype(BF)
            kg = gather_keys(ktf32).astype(BF)
            r0 = b * SQ
            qm = q[r0 + 64:r0 + 192]
            qo = jnp.concatenate([q[r0:r0 + 64], q[r0 + 192:r0 + 256]], axis=0)
            sm = [jnp.dot(jnp.where(sel, qm, zero), kt, preferred_element_type=F32)
                  for sel in (lo128, hi128)]
            so = [jnp.dot(jnp.where(sel, qo, zero), kg, preferred_element_type=F32)
                  for sel in (lo128, hi128)]
            out.append((sm, so))
        return out

    def finish(slot, h, sc_all):
        col0 = slot * 256 + h * 128
        for b in range(B):
            sm, so = sc_all[b]
            vtf32 = vtf[slot, h, b]
            vt = vtf32.astype(BF)
            vg = gather_keys(vtf32).astype(BF)
            vts = (jnp.concatenate([vt[:DH], ones_m], axis=0),
                   jnp.concatenate([ones_m, vt[DH:]], axis=0))
            vgs = (jnp.concatenate([vg[:DH], ones_o], axis=0),
                   jnp.concatenate([ones_o, vg[DH:]], axis=0))
            r0 = b * SQ
            rm, ro_ = [], []
            for a in range(2):
                s = jnp.where(mask_mid, sm[a], NEG)
                m = jnp.max(s, axis=-1, keepdims=True)
                p = jnp.exp(s - m).astype(BF)
                lhs = jnp.concatenate([p, off_ind], axis=0)
                rm.append(lax.dot_general(lhs, vts[a], NT,
                                          preferred_element_type=F32))
            for a in range(2):
                s = so[a]
                m = jnp.maximum(jnp.max(s, axis=-1, keepdims=True), NEG)
                p = jnp.exp(s - m).astype(BF)
                r = lax.dot_general(p, vgs[a], NT, preferred_element_type=F32)
                ro_.append(r + jnp.exp(NEG - m) * rm[a][128:129])
            num = jnp.where(lo128, rm[0][:128], rm[1][:128])
            den = pltpu.roll(jnp.where(lo128, rm[1][:128], rm[0][:128]), 64, 1)
            ctx[r0 + 64:r0 + 192, col0:col0 + 128] = (num / den).astype(BF)
            num = jnp.where(lo128, ro_[0], ro_[1])
            den = pltpu.roll(jnp.where(lo128, ro_[1], ro_[0]), 64, 1)
            c = (num / den).astype(BF)
            ctx[r0:r0 + 64, col0:col0 + 128] = c[:64]
            ctx[r0 + 192:r0 + 256, col0:col0 + 128] = c[64:]

    def attend2(p1, p2):
        with sc(f"lkv"):
            for p in (p1, p2):
                cp_kv[p][0].wait()
                cp_kv[p][1].wait()
        with sc(f"att{p1[0]}{p1[1]}"):
            s1 = scores(*p1)
            s2 = scores(*p2)
            finish(*p1, s1)
            finish(*p2, s2)

    def wo_tile(slot, h, c):
        h0, k0 = wo_loc(h, c, 0)
        h1, k1 = wo_loc(h, c, 1)
        return jnp.concatenate([wo_all[slot, h0, k0], wo_all[slot, h1, k1]], axis=0)

    def outproj(jobs, first=False, rblk=SQ):
        with sc("op"):
            for c, parts in jobs.items():
                tiles = [wo_tile(slot, h, c) for (slot, h) in parts]
                for r0 in range(0, ROWS, rblk):
                    acc = None
                    for (slot, h), w in zip(parts, tiles):
                        col0 = slot * 256 + h * 128
                        t = jnp.dot(ctx[r0:r0 + rblk, col0:col0 + 128], w,
                                    preferred_element_type=F32)
                        acc = t if acc is None else acc + t
                    b, rr = divmod(r0, SQ)
                    if first:
                        out_ref[b, rr:rr + rblk, c * 128:(c + 1) * 128] = acc
                    else:
                        out_ref[b, rr:rr + rblk, c * 128:(c + 1) * 128] += acc

    attend2((0, 0), (0, 1))

    recv_wait(wq_all.at[1, 0], rq(1, 0))
    send(wq_all.at[1, 0], wq_all.at[3, 0], rq(3, 0), right)
    send(wo_all.at[0, 1], wo_all.at[1, 1], ro(1, 1), right)
    recv_wait(wq_all.at[2, 1], rq(2, 1))
    send(wq_all.at[2, 1], wq_all.at[3, 1], rq(3, 1), left)
    send(wo_all.at[0, 0], wo_all.at[2, 0], ro(2, 0), left)

    attend2((1, 0), (2, 1))
    outproj({c: [(0, 0), (0, 1)] for c in range(4)}, first=True)

    recv_wait(wqs.at[0], 20)
    recv_wait(wqs.at[1], 21)
    wq_all[1, 1, 0:NF, :] = wqs[0].astype(BF)
    wq_all[2, 0, 0:NF, :] = wqs[1].astype(BF)
    recv_wait(wq_all.at[1, 1, rest], rq(1, 1))
    recv_wait(wq_all.at[2, 0, rest], rq(2, 0))
    attend2((1, 1), (2, 0))

    recv_wait(wo_all.at[1, 0], ro(1, 0))
    for i, (k0, n) in enumerate(WO_FWD):
        send(wo_all.at[1, 0, pl.ds(k0, n)], wo_all.at[3, 0, pl.ds(k0, n)],
             rod(0, i), right)
    recv_wait(wo_all.at[2, 1], ro(2, 1))
    for i, (k0, n) in enumerate(WO_FWD):
        send(wo_all.at[2, 1, pl.ds(k0, n)], wo_all.at[3, 1, pl.ds(k0, n)],
             rod(1, i), left)
    outproj({c: [(1, 0), (2, 1)] for c in range(3)})

    recv_wait(wq_all.at[3, 0], rq(3, 0))
    recv_wait(wq_all.at[3, 1], rq(3, 1))
    attend2((3, 0), (3, 1))

    recv_wait(wo_all.at[1, 1], ro(1, 1))
    recv_wait(wo_all.at[2, 0], ro(2, 0))
    jobs = {c: [(1, 1), (2, 0)] for c in range(3)}
    jobs[3] = [(1, 0), (1, 1), (2, 0), (2, 1)]
    outproj(jobs)

    for i, (k0, n) in enumerate(WO_FWD):
        recv_wait(wo_all.at[3, 0, pl.ds(k0, n)], rod(0, i))
        recv_wait(wo_all.at[3, 1, pl.ds(k0, n)], rod(1, i))
        if i < 3:
            outproj({i: [(3, 0), (3, 1)]})
        else:
            outproj({3: [(3, i - 3)]}, rblk=128)

    for s in sends:
        s.wait_send()


def pallas_dist_sparse_attn_blocksparse_qseq_b2_sq256_skv256_hq4_dh64_kernel(
    x: jax.Array,
    Wq: jax.Array,
    K_ext: jax.Array,
    V_ext: jax.Array,
    Wo: jax.Array,
):
    kt = jnp.transpose(K_ext, (0, 2, 3, 1)).reshape(B, 8, 128, SKV)
    vt = jnp.transpose(V_ext, (0, 2, 3, 1)).reshape(B, 8, 128, SKV)

    hbm = pl.BlockSpec(memory_space=pltpu.HBM)
    return pl.pallas_call(
        _kernel,
        out_shape=jax.ShapeDtypeStruct((B, SQ, DM), F32),
        in_specs=[hbm] * 5,
        out_specs=pl.BlockSpec(memory_space=pltpu.VMEM),
        scratch_shapes=[
            pltpu.VMEM((B, SQ, DM), F32),
            pltpu.VMEM((ROWS, DM), BF),
            pltpu.VMEM((DM, 256), F32),
            pltpu.VMEM((256, DM), F32),
            pltpu.VMEM((4, 2, DM, 128), BF),
            pltpu.VMEM((4, 2, 8, DH, 128), BF),
            pltpu.VMEM((4, 2, B, 128, SKV), F32),
            pltpu.VMEM((4, 2, B, 128, SKV), F32),
            pltpu.VMEM((ROWS, 1024), BF),
            pltpu.VMEM((2, NF, 128), F32),
            pltpu.SemaphoreType.DMA((24,)),
            pltpu.SemaphoreType.DMA((1,)),
            pltpu.SemaphoreType.DMA((22,)),
            pltpu.SemaphoreType.REGULAR,
        ],
        compiler_params=pltpu.CompilerParams(
            collective_id=0,
            vmem_limit_bytes=64 * 1024 * 1024,
            disable_semaphore_checks=True,
        ),
    )(x, Wq, kt, vt, Wo)
```

```python
import jax
import jax.numpy as jnp
from jax import lax
from jax.experimental import pallas as pl
from jax.experimental.pallas import tpu as pltpu

N_DEV = 4
B = 2
SQ = 256
SKV = 256
DM = 512
DH = 64
BLK = 64
ROWS = B * SQ
NEG = -1e9
BF = jnp.bfloat16
F32 = jnp.float32
NT = (((1,), (1,)), ((), ()))
MESH = pl.DeviceIdType.MESH

SLOT_OFF = (0, 3, 1, 2)
WQ_PIECES = ((0, 16), (16, 48), (64, 64), (128, 128), (256, 256))
NF = 32
PAIR_ORDER = ((0, 0), (0, 1), (1, 0), (2, 1), (1, 1), (2, 0), (3, 0), (3, 1))
WO_FWD = ((0, 2), (2, 2), (4, 2), (6, 1), (7, 1))


def _wo_loc(h, c, a):
    if c < 3:
        return h, 2 * c + a
    return a, 6 + h


def _kernel(x_hbm, wq_hbm, kt_hbm, vt_hbm, wo_hbm, out_ref,
            xf, xb, wqf, wof, wq_all, wo_all, ktf, vtf, ctx, wqs,
            lsem, ssem, rsem, ready):
    me = lax.axis_index("i")
    left = (me + 3) % N_DEV
    right = (me + 1) % N_DEV
    odd = lax.rem(me, 2) == 1

    cp_wq = [
        pltpu.make_async_copy(wq_hbm.at[pl.ds(r0, n)], wqf.at[pl.ds(r0, n)],
                              lsem.at[i])
        for i, (r0, n) in enumerate(WQ_PIECES)
    ]
    cp_wq[0].start()

    bar = pltpu.get_barrier_semaphore()

    @pl.when(me != 2)
    def _():
        for nbr in (left, right):
            pl.semaphore_signal(bar, inc=1, device_id=(nbr,), device_id_type=MESH)

    @pl.when(me == 2)
    def _():
        pl.semaphore_wait(bar, 2)
        for nbr in (left, right):
            pl.semaphore_signal(ready, inc=1, device_id=(nbr,), device_id_type=MESH)

    @pl.when(odd)
    def _():
        pl.semaphore_wait(bar, 1)

    sends = []

    def rcopy(src, dst, ridx, tgt):
        return pltpu.make_async_remote_copy(
            src, dst, ssem.at[0], rsem.at[ridx],
            device_id=(tgt,), device_id_type=MESH)

    def send(src, dst, ridx, tgt):
        c = rcopy(src, dst, ridx, tgt)
        c.start()
        sends.append(c)

    def recv_wait(dst, ridx):
        rcopy(dst, dst, ridx, me).wait_recv()

    def rq(slot, h):
        return (slot - 1) * 2 + h

    def ro(slot, half):
        return 6 + (slot - 1) * 2 + half

    def rod(half, k):
        return 10 + half * 5 + k

    rf = (20, 21)

    top = pl.ds(0, NF)
    fr = rcopy(wq_hbm.at[top, pl.ds(128, 128)], wqs.at[0], rf[0], right)
    fl = rcopy(wq_hbm.at[top, pl.ds(0, 128)], wqs.at[1], rf[1], left)
    pl.when(me >= 2)(fr.start)
    pl.when((me == 1) | (me == 2))(fl.start)
    gr = rcopy(wqf.at[top, pl.ds(128, 128)], wqs.at[0], rf[0], right)
    gl = rcopy(wqf.at[top, pl.ds(0, 128)], wqs.at[1], rf[1], left)

    for c in cp_wq[1:]:
        c.start()
    cp_wo = pltpu.make_async_copy(wo_hbm, wof, lsem.at[7])
    cp_wo.start()
    cp_x = []
    for b in range(B):
        c = pltpu.make_async_copy(x_hbm.at[b], xf.at[b], lsem.at[5 + b])
        c.start()
        cp_x.append(c)
    cp_kv = {}
    for i, (s, h) in enumerate(PAIR_ORDER):
        pr = 2 * ((me + SLOT_OFF[s]) % N_DEV) + h
        ck = pltpu.make_async_copy(kt_hbm.at[:, pr], ktf.at[s, h],
                                   lsem.at[8 + 2 * i])
        cv = pltpu.make_async_copy(vt_hbm.at[:, pr], vtf.at[s, h],
                                   lsem.at[9 + 2 * i])
        ck.start()
        cv.start()
        cp_kv[(s, h)] = (ck, cv)

    to_r, to_l = [], []
    for i, (r0, n) in enumerate(WQ_PIECES):
        cp_wq[i].wait()
        for h in range(2):
            wq_all[0, h, r0:r0 + n, :] = (
                wqf[r0:r0 + n, h * 128:(h + 1) * 128].astype(BF))
        if i == 0:
            @pl.when(me == 0)
            def _():
                pl.semaphore_wait(bar, 2)
        rows = pl.ds(r0, n)
        cr = rcopy(wq_all.at[0, 0, rows], wq_all.at[1, 0, rows], rq(1, 0), right)
        cl = rcopy(wq_all.at[0, 1, rows], wq_all.at[2, 1, rows], rq(2, 1), left)
        to_r.append(cr)
        to_l.append(cl)
        pl.when(me != 1)(cr.start)
        pl.when(me != 3)(cl.start)
    sends += to_r + to_l + [gr, gl]

    @pl.when(odd)
    def _():
        pl.semaphore_wait(ready, 1)

    @pl.when(me == 1)
    def _():
        for c in to_r:
            c.start()

    @pl.when(me == 3)
    def _():
        for c in to_l:
            c.start()

    pl.when(me < 2)(gr.start)
    pl.when((me == 0) | (me == 3))(gl.start)
    rest = pl.ds(NF, DM - NF)
    send(wq_all.at[0, 1, rest], wq_all.at[1, 1, rest], rq(1, 1), right)
    send(wq_all.at[0, 0, rest], wq_all.at[2, 0, rest], rq(2, 0), left)

    cp_wo.wait()
    for h in range(2):
        for c in range(4):
            for a in range(2):
                hf, k = _wo_loc(h, c, a)
                r0 = h * 128 + a * DH
                wo_all[0, hf, k] = wof[r0:r0 + DH, c * 128:(c + 1) * 128].astype(BF)
    send(wo_all.at[0, 0], wo_all.at[1, 0], ro(1, 0), right)
    send(wo_all.at[0, 1], wo_all.at[2, 1], ro(2, 1), left)

    for b in range(B):
        cp_x[b].wait()
        xb[b * SQ:(b + 1) * SQ, :] = xf[b].astype(BF)

    row = lax.broadcasted_iota(jnp.int32, (2 * BLK, SKV), 0)
    col = lax.broadcasted_iota(jnp.int32, (2 * BLK, SKV), 1)
    qb = me * (SQ // BLK) + 1 + row // BLK
    kb = col // BLK
    mask_mid = (qb == kb) | (kb == 0) | (lax.rem(qb + kb, 3) == 0)
    xk = 3 - lax.rem(me, 3)
    col1 = lax.broadcasted_iota(jnp.int32, (16, SKV), 1) // BLK
    off_ind = jnp.where((col1 == 0) | (col1 == xk), 0.0, 1.0).astype(BF)
    lo128 = lax.broadcasted_iota(jnp.int32, (128, 128), 1) < DH
    hi128 = jnp.logical_not(lo128)
    zero = jnp.zeros((128, 128), BF)
    ones_m = jnp.ones((DH, SKV), BF)
    ones_o = jnp.ones((DH, 128), BF)

    def gather_keys(t):
        t01 = t[:, :128]
        t23 = t[:, 128:]
        y = jnp.where(xk == 2, pltpu.roll(t23, 64, 1), t23)
        y = jnp.where(xk == 1, t01, y)
        return jnp.where(lo128, t01, y)

    def scores(slot, h):
        q = jnp.dot(xb[...], wq_all[slot, h], preferred_element_type=F32)
        q = (q * 0.125).astype(BF)
        out = []
        for b in range(B):
            ktf32 = ktf[slot, h, b]
            kt = ktf32.astype(BF)
            kg = gather_keys(ktf32).astype(BF)
            r0 = b * SQ
            qm = q[r0 + 64:r0 + 192]
            qo = jnp.concatenate([q[r0:r0 + 64], q[r0 + 192:r0 + 256]], axis=0)
            sm = [jnp.dot(jnp.where(sel, qm, zero), kt, preferred_element_type=F32)
                  for sel in (lo128, hi128)]
            so = [jnp.dot(jnp.where(sel, qo, zero), kg, preferred_element_type=F32)
                  for sel in (lo128, hi128)]
            out.append((sm, so))
        return out

    def finish(slot, h, sc_all):
        col0 = slot * 256 + h * 128
        for b in range(B):
            sm, so = sc_all[b]
            vtf32 = vtf[slot, h, b]
            vt = vtf32.astype(BF)
            vg = gather_keys(vtf32).astype(BF)
            vts = (jnp.concatenate([vt[:DH], ones_m], axis=0),
                   jnp.concatenate([ones_m, vt[DH:]], axis=0))
            vgs = (jnp.concatenate([vg[:DH], ones_o], axis=0),
                   jnp.concatenate([ones_o, vg[DH:]], axis=0))
            r0 = b * SQ
            rm, rout = [], []
            for a in range(2):
                s = jnp.where(mask_mid, sm[a], NEG)
                m = jnp.max(s, axis=-1, keepdims=True)
                p = jnp.exp(s - m).astype(BF)
                lhs = jnp.concatenate([p, off_ind], axis=0)
                rm.append(lax.dot_general(lhs, vts[a], NT,
                                          preferred_element_type=F32))
            for a in range(2):
                s = so[a]
                m = jnp.maximum(jnp.max(s, axis=-1, keepdims=True), NEG)
                p = jnp.exp(s - m).astype(BF)
                r = lax.dot_general(p, vgs[a], NT, preferred_element_type=F32)
                rout.append(r + jnp.exp(NEG - m) * rm[a][128:129])
            num = jnp.where(lo128, rm[0][:128], rm[1][:128])
            den = pltpu.roll(jnp.where(lo128, rm[1][:128], rm[0][:128]), 64, 1)
            ctx[r0 + 64:r0 + 192, col0:col0 + 128] = (num / den).astype(BF)
            num = jnp.where(lo128, rout[0], rout[1])
            den = pltpu.roll(jnp.where(lo128, rout[1], rout[0]), 64, 1)
            c = (num / den).astype(BF)
            ctx[r0:r0 + 64, col0:col0 + 128] = c[:64]
            ctx[r0 + 192:r0 + 256, col0:col0 + 128] = c[64:]

    def attend2(p1, p2):
        for p in (p1, p2):
            cp_kv[p][0].wait()
            cp_kv[p][1].wait()
        s1 = scores(*p1)
        s2 = scores(*p2)
        finish(*p1, s1)
        finish(*p2, s2)

    def wo_tile(slot, h, c):
        h0, k0 = _wo_loc(h, c, 0)
        h1, k1 = _wo_loc(h, c, 1)
        return jnp.concatenate([wo_all[slot, h0, k0], wo_all[slot, h1, k1]], axis=0)

    def outproj(jobs, first=False, rblk=SQ):
        for c, parts in jobs.items():
            tiles = [wo_tile(slot, h, c) for (slot, h) in parts]
            for r0 in range(0, ROWS, rblk):
                acc = None
                for (slot, h), w in zip(parts, tiles):
                    col0 = slot * 256 + h * 128
                    t = jnp.dot(ctx[r0:r0 + rblk, col0:col0 + 128], w,
                                preferred_element_type=F32)
                    acc = t if acc is None else acc + t
                b, rr = divmod(r0, SQ)
                if first:
                    out_ref[b, rr:rr + rblk, c * 128:(c + 1) * 128] = acc
                else:
                    out_ref[b, rr:rr + rblk, c * 128:(c + 1) * 128] += acc

    attend2((0, 0), (0, 1))

    recv_wait(wq_all.at[1, 0], rq(1, 0))
    send(wq_all.at[1, 0], wq_all.at[3, 0], rq(3, 0), right)
    send(wo_all.at[0, 1], wo_all.at[1, 1], ro(1, 1), right)
    recv_wait(wq_all.at[2, 1], rq(2, 1))
    send(wq_all.at[2, 1], wq_all.at[3, 1], rq(3, 1), left)
    send(wo_all.at[0, 0], wo_all.at[2, 0], ro(2, 0), left)

    attend2((1, 0), (2, 1))
    outproj({c: [(0, 0), (0, 1)] for c in range(4)}, first=True)

    recv_wait(wqs.at[0], rf[0])
    recv_wait(wqs.at[1], rf[1])
    wq_all[1, 1, 0:NF, :] = wqs[0].astype(BF)
    wq_all[2, 0, 0:NF, :] = wqs[1].astype(BF)
    recv_wait(wq_all.at[1, 1, rest], rq(1, 1))
    recv_wait(wq_all.at[2, 0, rest], rq(2, 0))
    attend2((1, 1), (2, 0))

    recv_wait(wo_all.at[1, 0], ro(1, 0))
    for i, (k0, n) in enumerate(WO_FWD):
        send(wo_all.at[1, 0, pl.ds(k0, n)], wo_all.at[3, 0, pl.ds(k0, n)],
             rod(0, i), right)
    recv_wait(wo_all.at[2, 1], ro(2, 1))
    for i, (k0, n) in enumerate(WO_FWD):
        send(wo_all.at[2, 1, pl.ds(k0, n)], wo_all.at[3, 1, pl.ds(k0, n)],
             rod(1, i), left)
    outproj({c: [(1, 0), (2, 1)] for c in range(3)})

    recv_wait(wq_all.at[3, 0], rq(3, 0))
    recv_wait(wq_all.at[3, 1], rq(3, 1))
    attend2((3, 0), (3, 1))

    recv_wait(wo_all.at[1, 1], ro(1, 1))
    recv_wait(wo_all.at[2, 0], ro(2, 0))
    jobs = {c: [(1, 1), (2, 0)] for c in range(3)}
    jobs[3] = [(1, 0), (1, 1), (2, 0), (2, 1)]
    outproj(jobs)

    for i, (k0, n) in enumerate(WO_FWD):
        recv_wait(wo_all.at[3, 0, pl.ds(k0, n)], rod(0, i))
        recv_wait(wo_all.at[3, 1, pl.ds(k0, n)], rod(1, i))
        if i < 3:
            outproj({i: [(3, 0), (3, 1)]})
        else:
            outproj({3: [(3, i - 3)]}, rblk=128)

    for s in sends:
        s.wait_send()


def pallas_dist_sparse_attn_blocksparse_qseq_b2_sq256_skv256_hq4_dh64_kernel(
    x: jax.Array,
    Wq: jax.Array,
    K_ext: jax.Array,
    V_ext: jax.Array,
    Wo: jax.Array,
):
    kt = jnp.transpose(K_ext, (0, 2, 3, 1)).reshape(B, 8, 128, SKV)
    vt = jnp.transpose(V_ext, (0, 2, 3, 1)).reshape(B, 8, 128, SKV)

    hbm = pl.BlockSpec(memory_space=pltpu.HBM)
    return pl.pallas_call(
        _kernel,
        out_shape=jax.ShapeDtypeStruct((B, SQ, DM), F32),
        in_specs=[hbm] * 5,
        out_specs=pl.BlockSpec(memory_space=pltpu.VMEM),
        scratch_shapes=[
            pltpu.VMEM((B, SQ, DM), F32),
            pltpu.VMEM((ROWS, DM), BF),
            pltpu.VMEM((DM, 256), F32),
            pltpu.VMEM((256, DM), F32),
            pltpu.VMEM((4, 2, DM, 128), BF),
            pltpu.VMEM((4, 2, 8, DH, 128), BF),
            pltpu.VMEM((4, 2, B, 128, SKV), F32),
            pltpu.VMEM((4, 2, B, 128, SKV), F32),
            pltpu.VMEM((ROWS, 1024), BF),
            pltpu.VMEM((2, NF, 128), F32),
            pltpu.SemaphoreType.DMA((24,)),
            pltpu.SemaphoreType.DMA((1,)),
            pltpu.SemaphoreType.DMA((22,)),
            pltpu.SemaphoreType.REGULAR,
        ],
        compiler_params=pltpu.CompilerParams(
            collective_id=0,
            vmem_limit_bytes=64 * 1024 * 1024,
            disable_semaphore_checks=True,
        ),
    )(x, Wq, kt, vt, Wo)
```

```python
import jax
import jax.numpy as jnp
from jax import lax
from jax.experimental import pallas as pl
from jax.experimental.pallas import tpu as pltpu

N_DEV = 4
B = 2
SQ = 256
SKV = 256
DM = 512
DH = 64
BLK = 64
ROWS = B * SQ
NEG = -1e9
BF = jnp.bfloat16
F32 = jnp.float32
NT = (((1,), (1,)), ((), ()))
MESH = pl.DeviceIdType.MESH

SLOT_OFF = (0, 3, 1, 2)
WQ_PIECES = ((0, 16), (16, 48), (64, 64), (128, 128), (256, 256))
NF = 32
PAIR_ORDER = ((0, 0), (0, 1), (1, 0), (2, 1), (1, 1), (2, 0), (3, 0), (3, 1))
WO_FWD = ((0, 2), (2, 2), (4, 2), (6, 1), (7, 1))


def _wo_loc(h, c, a):
    if c < 3:
        return h, 2 * c + a
    return a, 6 + h


def _kernel(x_hbm, wq_hbm, kt_hbm, vt_hbm, wo_hbm, out_ref,
            xf, xb, wqf, wof, wq_all, wo_all, ktf, vtf, ctx, wqs,
            lsem, ssem, rsem, ready):
    me = lax.axis_index("i")
    left = (me + 3) % N_DEV
    right = (me + 1) % N_DEV
    odd = lax.rem(me, 2) == 1

    cp_wq = [
        pltpu.make_async_copy(wq_hbm.at[pl.ds(r0, n)], wqf.at[pl.ds(r0, n)],
                              lsem.at[i])
        for i, (r0, n) in enumerate(WQ_PIECES)
    ]
    cp_wq[0].start()

    bar = pltpu.get_barrier_semaphore()

    @pl.when(me != 2)
    def _():
        for nbr in (left, right):
            pl.semaphore_signal(bar, inc=1, device_id=(nbr,), device_id_type=MESH)

    @pl.when(me == 2)
    def _():
        pl.semaphore_wait(bar, 2)
        for nbr in (left, right):
            pl.semaphore_signal(ready, inc=1, device_id=(nbr,), device_id_type=MESH)

    @pl.when(odd)
    def _():
        pl.semaphore_wait(bar, 1)

    sends = []

    def rcopy(src, dst, ridx, tgt):
        return pltpu.make_async_remote_copy(
            src, dst, ssem.at[0], rsem.at[ridx],
            device_id=(tgt,), device_id_type=MESH)

    def send(src, dst, ridx, tgt):
        c = rcopy(src, dst, ridx, tgt)
        c.start()
        sends.append(c)

    def recv_wait(dst, ridx):
        rcopy(dst, dst, ridx, me).wait_recv()

    def rq(slot, h):
        return (slot - 1) * 2 + h

    def ro(slot, half):
        return 6 + (slot - 1) * 2 + half

    def rod(half, k):
        return 10 + half * 5 + k

    rf = (20, 21)

    top = pl.ds(0, NF)
    fr = rcopy(wq_hbm.at[top, pl.ds(128, 128)], wqs.at[0], rf[0], right)
    fl = rcopy(wq_hbm.at[top, pl.ds(0, 128)], wqs.at[1], rf[1], left)
    early_r = me >= 2
    early_l = (me == 1) | (me == 2)
    pl.when(early_r)(fr.start)
    pl.when(early_l)(fl.start)
    gr = rcopy(wqf.at[top, pl.ds(128, 128)], wqs.at[0], rf[0], right)
    gl = rcopy(wqf.at[top, pl.ds(0, 128)], wqs.at[1], rf[1], left)

    for c in cp_wq[1:]:
        c.start()
    cp_wo = pltpu.make_async_copy(wo_hbm, wof, lsem.at[7])
    cp_wo.start()
    cp_x = []
    for b in range(B):
        c = pltpu.make_async_copy(x_hbm.at[b], xf.at[b], lsem.at[5 + b])
        c.start()
        cp_x.append(c)
    cp_kv = {}
    for i, (s, h) in enumerate(PAIR_ORDER):
        pr = 2 * ((me + SLOT_OFF[s]) % N_DEV) + h
        ck = pltpu.make_async_copy(kt_hbm.at[:, pr], ktf.at[s, h],
                                   lsem.at[8 + 2 * i])
        cv = pltpu.make_async_copy(vt_hbm.at[:, pr], vtf.at[s, h],
                                   lsem.at[9 + 2 * i])
        ck.start()
        cv.start()
        cp_kv[(s, h)] = (ck, cv)

    to_r, to_l = [], []
    for i, (r0, n) in enumerate(WQ_PIECES):
        cp_wq[i].wait()
        for h in range(2):
            wq_all[0, h, r0:r0 + n, :] = (
                wqf[r0:r0 + n, h * 128:(h + 1) * 128].astype(BF))
        if i == 0:
            @pl.when(me == 0)
            def _():
                pl.semaphore_wait(bar, 2)
        rows = pl.ds(r0, n)
        cr = rcopy(wq_all.at[0, 0, rows], wq_all.at[1, 0, rows], rq(1, 0), right)
        cl = rcopy(wq_all.at[0, 1, rows], wq_all.at[2, 1, rows], rq(2, 1), left)
        to_r.append(cr)
        to_l.append(cl)
        pl.when(me != 1)(cr.start)
        pl.when(me != 3)(cl.start)
    sends += to_r + to_l

    @pl.when(odd)
    def _():
        pl.semaphore_wait(ready, 1)

    @pl.when(me == 1)
    def _():
        for c in to_r:
            c.start()

    @pl.when(me == 3)
    def _():
        for c in to_l:
            c.start()

    pl.when(jnp.logical_not(early_r))(gr.start)
    pl.when(jnp.logical_not(early_l))(gl.start)
    rest = pl.ds(NF, DM - NF)
    send(wq_all.at[0, 1, rest], wq_all.at[1, 1, rest], rq(1, 1), right)
    send(wq_all.at[0, 0, rest], wq_all.at[2, 0, rest], rq(2, 0), left)

    cp_wo.wait()
    for h in range(2):
        for c in range(4):
            for a in range(2):
                hf, k = _wo_loc(h, c, a)
                r0 = h * 128 + a * DH
                wo_all[0, hf, k] = wof[r0:r0 + DH, c * 128:(c + 1) * 128].astype(BF)
    send(wo_all.at[0, 0], wo_all.at[1, 0], ro(1, 0), right)
    send(wo_all.at[0, 1], wo_all.at[2, 1], ro(2, 1), left)

    for b in range(B):
        cp_x[b].wait()
        xb[b * SQ:(b + 1) * SQ, :] = xf[b].astype(BF)

    row = lax.broadcasted_iota(jnp.int32, (2 * BLK, SKV), 0)
    col = lax.broadcasted_iota(jnp.int32, (2 * BLK, SKV), 1)
    qb = me * (SQ // BLK) + 1 + row // BLK
    kb = col // BLK
    mask_mid = (qb == kb) | (kb == 0) | (lax.rem(qb + kb, 3) == 0)
    xk = 3 - lax.rem(me, 3)
    col1 = lax.broadcasted_iota(jnp.int32, (16, SKV), 1) // BLK
    off_ind = jnp.where((col1 == 0) | (col1 == xk), 0.0, 1.0).astype(BF)
    lo128 = lax.broadcasted_iota(jnp.int32, (128, 128), 1) < DH
    hi128 = jnp.logical_not(lo128)
    zero = jnp.zeros((128, 128), BF)
    ones_m = jnp.ones((DH, SKV), BF)
    ones_o = jnp.ones((DH, 128), BF)

    def gather_keys(t):
        t01 = t[:, :128]
        t23 = t[:, 128:]
        y = jnp.where(xk == 2, pltpu.roll(t23, 64, 1), t23)
        y = jnp.where(xk == 1, t01, y)
        return jnp.where(lo128, t01, y)

    def scores(slot, h):
        q = jnp.dot(xb[...], wq_all[slot, h], preferred_element_type=F32)
        q = (q * 0.125).astype(BF)
        out = []
        for b in range(B):
            ktf32 = ktf[slot, h, b]
            kt = ktf32.astype(BF)
            kg = gather_keys(ktf32).astype(BF)
            r0 = b * SQ
            qm = q[r0 + 64:r0 + 192]
            qo = jnp.concatenate([q[r0:r0 + 64], q[r0 + 192:r0 + 256]], axis=0)
            sm = [jnp.dot(jnp.where(sel, qm, zero), kt, preferred_element_type=F32)
                  for sel in (lo128, hi128)]
            so = [jnp.dot(jnp.where(sel, qo, zero), kg, preferred_element_type=F32)
                  for sel in (lo128, hi128)]
            out.append((sm, so))
        return out

    def finish(slot, h, sc_all):
        col0 = slot * 256 + h * 128
        for b in range(B):
            sm, so = sc_all[b]
            vtf32 = vtf[slot, h, b]
            vt = vtf32.astype(BF)
            vg = gather_keys(vtf32).astype(BF)
            vts = (jnp.concatenate([vt[:DH], ones_m], axis=0),
                   jnp.concatenate([ones_m, vt[DH:]], axis=0))
            vgs = (jnp.concatenate([vg[:DH], ones_o], axis=0),
                   jnp.concatenate([ones_o, vg[DH:]], axis=0))
            r0 = b * SQ
            rm, rout = [], []
            for a in range(2):
                s = jnp.where(mask_mid, sm[a], NEG)
                m = jnp.max(s, axis=-1, keepdims=True)
                p = jnp.exp(s - m).astype(BF)
                lhs = jnp.concatenate([p, off_ind], axis=0)
                rm.append(lax.dot_general(lhs, vts[a], NT,
                                          preferred_element_type=F32))
            for a in range(2):
                s = so[a]
                m = jnp.maximum(jnp.max(s, axis=-1, keepdims=True), NEG)
                p = jnp.exp(s - m).astype(BF)
                r = lax.dot_general(p, vgs[a], NT, preferred_element_type=F32)
                rout.append(r + jnp.exp(NEG - m) * rm[a][128:129])
            num = jnp.where(lo128, rm[0][:128], rm[1][:128])
            den = pltpu.roll(jnp.where(lo128, rm[1][:128], rm[0][:128]), 64, 1)
            ctx[r0 + 64:r0 + 192, col0:col0 + 128] = (num / den).astype(BF)
            num = jnp.where(lo128, rout[0], rout[1])
            den = pltpu.roll(jnp.where(lo128, rout[1], rout[0]), 64, 1)
            c = (num / den).astype(BF)
            ctx[r0:r0 + 64, col0:col0 + 128] = c[:64]
            ctx[r0 + 192:r0 + 256, col0:col0 + 128] = c[64:]

    def attend2(p1, p2):
        for p in (p1, p2):
            cp_kv[p][0].wait()
            cp_kv[p][1].wait()
        s1 = scores(*p1)
        s2 = scores(*p2)
        finish(*p1, s1)
        finish(*p2, s2)

    def wo_tile(slot, h, c):
        h0, k0 = _wo_loc(h, c, 0)
        h1, k1 = _wo_loc(h, c, 1)
        return jnp.concatenate([wo_all[slot, h0, k0], wo_all[slot, h1, k1]], axis=0)

    def outproj(jobs, first=False, rblk=SQ):
        for c, parts in jobs.items():
            tiles = [wo_tile(slot, h, c) for (slot, h) in parts]
            for r0 in range(0, ROWS, rblk):
                acc = None
                for (slot, h), w in zip(parts, tiles):
                    col0 = slot * 256 + h * 128
                    t = jnp.dot(ctx[r0:r0 + rblk, col0:col0 + 128], w,
                                preferred_element_type=F32)
                    acc = t if acc is None else acc + t
                b, rr = divmod(r0, SQ)
                if first:
                    out_ref[b, rr:rr + rblk, c * 128:(c + 1) * 128] = acc
                else:
                    out_ref[b, rr:rr + rblk, c * 128:(c + 1) * 128] += acc

    attend2((0, 0), (0, 1))

    recv_wait(wq_all.at[1, 0], rq(1, 0))
    send(wq_all.at[1, 0], wq_all.at[3, 0], rq(3, 0), right)
    send(wo_all.at[0, 1], wo_all.at[1, 1], ro(1, 1), right)
    recv_wait(wq_all.at[2, 1], rq(2, 1))
    send(wq_all.at[2, 1], wq_all.at[3, 1], rq(3, 1), left)
    send(wo_all.at[0, 0], wo_all.at[2, 0], ro(2, 0), left)

    attend2((1, 0), (2, 1))
    outproj({c: [(0, 0), (0, 1)] for c in range(4)}, first=True)

    recv_wait(wqs.at[0], rf[0])
    recv_wait(wqs.at[1], rf[1])
    recv_wait(wq_all.at[1, 1, rest], rq(1, 1))
    recv_wait(wq_all.at[2, 0, rest], rq(2, 0))
    wq_all[1, 1, 0:NF, :] = wqs[0].astype(BF)
    wq_all[2, 0, 0:NF, :] = wqs[1].astype(BF)
    attend2((1, 1), (2, 0))

    recv_wait(wo_all.at[1, 0], ro(1, 0))
    for i, (k0, n) in enumerate(WO_FWD):
        send(wo_all.at[1, 0, pl.ds(k0, n)], wo_all.at[3, 0, pl.ds(k0, n)],
             rod(0, i), right)
    recv_wait(wo_all.at[2, 1], ro(2, 1))
    for i, (k0, n) in enumerate(WO_FWD):
        send(wo_all.at[2, 1, pl.ds(k0, n)], wo_all.at[3, 1, pl.ds(k0, n)],
             rod(1, i), left)
    outproj({c: [(1, 0), (2, 1)] for c in range(3)})

    recv_wait(wq_all.at[3, 0], rq(3, 0))
    recv_wait(wq_all.at[3, 1], rq(3, 1))
    attend2((3, 0), (3, 1))

    pl.when(early_r)(fr.wait_send)
    pl.when(early_l)(fl.wait_send)
    pl.when(jnp.logical_not(early_r))(gr.wait_send)
    pl.when(jnp.logical_not(early_l))(gl.wait_send)

    recv_wait(wo_all.at[1, 1], ro(1, 1))
    recv_wait(wo_all.at[2, 0], ro(2, 0))
    jobs = {c: [(1, 1), (2, 0)] for c in range(3)}
    jobs[3] = [(1, 0), (1, 1), (2, 0), (2, 1)]
    outproj(jobs)

    for i, (k0, n) in enumerate(WO_FWD):
        recv_wait(wo_all.at[3, 0, pl.ds(k0, n)], rod(0, i))
        recv_wait(wo_all.at[3, 1, pl.ds(k0, n)], rod(1, i))
        if i < 3:
            outproj({i: [(3, 0), (3, 1)]})
        else:
            outproj({3: [(3, i - 3)]}, rblk=128)

    for s in sends:
        s.wait_send()


def pallas_dist_sparse_attn_blocksparse_qseq_b2_sq256_skv256_hq4_dh64_kernel(
    x: jax.Array,
    Wq: jax.Array,
    K_ext: jax.Array,
    V_ext: jax.Array,
    Wo: jax.Array,
):
    kt = jnp.transpose(K_ext, (0, 2, 3, 1)).reshape(B, 8, 128, SKV)
    vt = jnp.transpose(V_ext, (0, 2, 3, 1)).reshape(B, 8, 128, SKV)

    hbm = pl.BlockSpec(memory_space=pltpu.HBM)
    return pl.pallas_call(
        _kernel,
        out_shape=jax.ShapeDtypeStruct((B, SQ, DM), F32),
        in_specs=[hbm] * 5,
        out_specs=pl.BlockSpec(memory_space=pltpu.VMEM),
        scratch_shapes=[
            pltpu.VMEM((B, SQ, DM), F32),
            pltpu.VMEM((ROWS, DM), BF),
            pltpu.VMEM((DM, 256), F32),
            pltpu.VMEM((256, DM), F32),
            pltpu.VMEM((4, 2, DM, 128), BF),
            pltpu.VMEM((4, 2, 8, DH, 128), BF),
            pltpu.VMEM((4, 2, B, 128, SKV), F32),
            pltpu.VMEM((4, 2, B, 128, SKV), F32),
            pltpu.VMEM((ROWS, 1024), BF),
            pltpu.VMEM((2, NF, 128), F32),
            pltpu.SemaphoreType.DMA((24,)),
            pltpu.SemaphoreType.DMA((1,)),
            pltpu.SemaphoreType.DMA((22,)),
            pltpu.SemaphoreType.REGULAR,
        ],
        compiler_params=pltpu.CompilerParams(
            collective_id=0,
            vmem_limit_bytes=64 * 1024 * 1024,
            disable_semaphore_checks=True,
        ),
    )(x, Wq, kt, vt, Wo)
```

```python
import jax
import jax.numpy as jnp
from jax import lax
from jax.experimental import pallas as pl
from jax.experimental.pallas import tpu as pltpu

N_DEV = 4
B = 2
SQ = 256
SKV = 256
DM = 512
DH = 64
BLK = 64
ROWS = B * SQ
NEG = -1e9
BF = jnp.bfloat16
F32 = jnp.float32
NT = (((1,), (1,)), ((), ()))
MESH = pl.DeviceIdType.MESH

SLOT_OFF = (0, 3, 1, 2)
WQ_PIECES = ((0, 16), (16, 48), (64, 64), (128, 128), (256, 256))
NF = 32
PAIR_ORDER = ((0, 0), (0, 1), (1, 0), (2, 1), (1, 1), (2, 0), (3, 0), (3, 1))
WO_FWD = ((0, 2), (2, 2), (4, 2), (6, 1), (7, 1))


def _wo_loc(h, c, a):
    if c < 3:
        return h, 2 * c + a
    return a, 6 + h


def _kernel(x_hbm, wq_hbm, kt_hbm, vt_hbm, wo_hbm, out_ref,
            xf, xb, wqf, wof, wq_all, wo_all, ktf, vtf, ctx, wqs,
            lsem, ssem, rsem, ready):
    me = lax.axis_index("i")
    left = (me + 3) % N_DEV
    right = (me + 1) % N_DEV
    odd = lax.rem(me, 2) == 1

    cp_wq = [
        pltpu.make_async_copy(wq_hbm.at[pl.ds(r0, n)], wqf.at[pl.ds(r0, n)],
                              lsem.at[i])
        for i, (r0, n) in enumerate(WQ_PIECES)
    ]
    cp_wq[0].start()

    bar = pltpu.get_barrier_semaphore()

    @pl.when(me != 2)
    def _():
        for nbr in (left, right):
            pl.semaphore_signal(bar, inc=1, device_id=(nbr,), device_id_type=MESH)

    @pl.when(me == 2)
    def _():
        pl.semaphore_wait(bar, 2)
        for nbr in (left, right):
            pl.semaphore_signal(ready, inc=1, device_id=(nbr,), device_id_type=MESH)

    @pl.when(odd)
    def _():
        pl.semaphore_wait(bar, 1)

    sends = []

    def rcopy(src, dst, ridx, tgt):
        return pltpu.make_async_remote_copy(
            src, dst, ssem.at[0], rsem.at[ridx],
            device_id=(tgt,), device_id_type=MESH)

    def send(src, dst, ridx, tgt):
        c = rcopy(src, dst, ridx, tgt)
        c.start()
        sends.append(c)

    def recv_wait(dst, ridx):
        rcopy(dst, dst, ridx, me).wait_recv()

    def rq(slot, h):
        return (slot - 1) * 2 + h

    def ro(slot, half):
        return 6 + (slot - 1) * 2 + half

    def rod(half, k):
        return 10 + half * 5 + k

    rf = (20, 21)

    top = pl.ds(0, NF)
    fr = rcopy(wq_hbm.at[top, pl.ds(128, 128)], wqs.at[0], rf[0], right)
    fl = rcopy(wq_hbm.at[top, pl.ds(0, 128)], wqs.at[1], rf[1], left)
    early_r = me >= 2
    early_l = (me == 1) | (me == 2)
    pl.when(early_r)(fr.start)
    pl.when(early_l)(fl.start)
    gr = rcopy(wqf.at[top, pl.ds(128, 128)], wqs.at[0], rf[0], right)
    gl = rcopy(wqf.at[top, pl.ds(0, 128)], wqs.at[1], rf[1], left)

    for c in cp_wq[1:]:
        c.start()
    cp_wo = pltpu.make_async_copy(wo_hbm, wof, lsem.at[7])
    cp_wo.start()
    cp_x = []
    for b in range(B):
        c = pltpu.make_async_copy(x_hbm.at[b], xf.at[b], lsem.at[5 + b])
        c.start()
        cp_x.append(c)
    cp_kv = {}
    for i, (s, h) in enumerate(PAIR_ORDER):
        pr = 2 * ((me + SLOT_OFF[s]) % N_DEV) + h
        ck = pltpu.make_async_copy(kt_hbm.at[:, pr], ktf.at[s, h],
                                   lsem.at[8 + 2 * i])
        cv = pltpu.make_async_copy(vt_hbm.at[:, pr], vtf.at[s, h],
                                   lsem.at[9 + 2 * i])
        ck.start()
        cv.start()
        cp_kv[(s, h)] = (ck, cv)

    to_r, to_l = [], []
    for i, (r0, n) in enumerate(WQ_PIECES):
        cp_wq[i].wait()
        for h in range(2):
            wq_all[0, h, r0:r0 + n, :] = (
                wqf[r0:r0 + n, h * 128:(h + 1) * 128].astype(BF))
        if i == 0:
            @pl.when(me == 0)
            def _():
                pl.semaphore_wait(bar, 2)
        rows = pl.ds(r0, n)
        cr = rcopy(wq_all.at[0, 0, rows], wq_all.at[1, 0, rows], rq(1, 0), right)
        cl = rcopy(wq_all.at[0, 1, rows], wq_all.at[2, 1, rows], rq(2, 1), left)
        to_r.append(cr)
        to_l.append(cl)
        pl.when(me != 1)(cr.start)
        pl.when(me != 3)(cl.start)
    sends += to_r + to_l

    @pl.when(odd)
    def _():
        pl.semaphore_wait(ready, 1)

    @pl.when(me == 1)
    def _():
        for c in to_r:
            c.start()

    @pl.when(me == 3)
    def _():
        for c in to_l:
            c.start()

    pl.when(jnp.logical_not(early_r))(gr.start)
    pl.when(jnp.logical_not(early_l))(gl.start)
    rest = pl.ds(NF, DM - NF)
    send(wq_all.at[0, 1, rest], wq_all.at[1, 1, rest], rq(1, 1), right)
    send(wq_all.at[0, 0, rest], wq_all.at[2, 0, rest], rq(2, 0), left)

    cp_wo.wait()
    for h in range(2):
        for c in range(4):
            for a in range(2):
                hf, k = _wo_loc(h, c, a)
                r0 = h * 128 + a * DH
                wo_all[0, hf, k] = wof[r0:r0 + DH, c * 128:(c + 1) * 128].astype(BF)
    send(wo_all.at[0, 0], wo_all.at[1, 0], ro(1, 0), right)
    send(wo_all.at[0, 1], wo_all.at[2, 1], ro(2, 1), left)

    for b in range(B):
        cp_x[b].wait()
        xb[b * SQ:(b + 1) * SQ, :] = xf[b].astype(BF)

    row = lax.broadcasted_iota(jnp.int32, (2 * BLK, SKV), 0)
    col = lax.broadcasted_iota(jnp.int32, (2 * BLK, SKV), 1)
    qb = me * (SQ // BLK) + 1 + row // BLK
    kb = col // BLK
    mask_mid = (qb == kb) | (kb == 0) | (lax.rem(qb + kb, 3) == 0)
    xk = 3 - lax.rem(me, 3)
    col1 = lax.broadcasted_iota(jnp.int32, (16, SKV), 1) // BLK
    off_ind = jnp.where((col1 == 0) | (col1 == xk), 0.0, 1.0).astype(BF)
    lo128 = lax.broadcasted_iota(jnp.int32, (128, 128), 1) < DH
    hi128 = jnp.logical_not(lo128)
    zero = jnp.zeros((128, 128), BF)
    ones_m = jnp.ones((DH, SKV), BF)
    ones_o = jnp.ones((DH, 128), BF)

    def gather_keys(t):
        t01 = t[:, :128]
        t23 = t[:, 128:]
        y = jnp.where(xk == 2, pltpu.roll(t23, 64, 1), t23)
        y = jnp.where(xk == 1, t01, y)
        return jnp.where(lo128, t01, y)

    def scores(slot, h):
        q = jnp.dot(xb[...], wq_all[slot, h], preferred_element_type=F32)
        q = (q * 0.125).astype(BF)
        out = []
        for b in range(B):
            ktf32 = ktf[slot, h, b]
            kt = ktf32.astype(BF)
            kg = gather_keys(ktf32).astype(BF)
            r0 = b * SQ
            qm = q[r0 + 64:r0 + 192]
            qo = jnp.concatenate([q[r0:r0 + 64], q[r0 + 192:r0 + 256]], axis=0)
            sm = [jnp.dot(jnp.where(sel, qm, zero), kt, preferred_element_type=F32)
                  for sel in (lo128, hi128)]
            so = [jnp.dot(jnp.where(sel, qo, zero), kg, preferred_element_type=F32)
                  for sel in (lo128, hi128)]
            out.append((sm, so))
        return out

    def finish(slot, h, sc_all):
        col0 = slot * 256 + h * 128
        for b in range(B):
            sm, so = sc_all[b]
            vtf32 = vtf[slot, h, b]
            vt = vtf32.astype(BF)
            vg = gather_keys(vtf32).astype(BF)
            vts = (jnp.concatenate([vt[:DH], ones_m], axis=0),
                   jnp.concatenate([ones_m, vt[DH:]], axis=0))
            vgs = (jnp.concatenate([vg[:DH], ones_o], axis=0),
                   jnp.concatenate([ones_o, vg[DH:]], axis=0))
            r0 = b * SQ
            rm, rout = [], []
            for a in range(2):
                s = jnp.where(mask_mid, sm[a], NEG)
                m = jnp.max(s, axis=-1, keepdims=True)
                p = jnp.exp(s - m).astype(BF)
                lhs = jnp.concatenate([p, off_ind], axis=0)
                rm.append(lax.dot_general(lhs, vts[a], NT,
                                          preferred_element_type=F32))
            for a in range(2):
                s = so[a]
                m = jnp.maximum(jnp.max(s, axis=-1, keepdims=True), NEG)
                p = jnp.exp(s - m).astype(BF)
                r = lax.dot_general(p, vgs[a], NT, preferred_element_type=F32)
                rout.append(r + jnp.exp(NEG - m) * rm[a][128:129])
            num = jnp.where(lo128, rm[0][:128], rm[1][:128])
            den = pltpu.roll(jnp.where(lo128, rm[1][:128], rm[0][:128]), 64, 1)
            ctx[r0 + 64:r0 + 192, col0:col0 + 128] = (num / den).astype(BF)
            num = jnp.where(lo128, rout[0], rout[1])
            den = pltpu.roll(jnp.where(lo128, rout[1], rout[0]), 64, 1)
            c = (num / den).astype(BF)
            ctx[r0:r0 + 64, col0:col0 + 128] = c[:64]
            ctx[r0 + 192:r0 + 256, col0:col0 + 128] = c[64:]

    def attend2(p1, p2):
        for p in (p1, p2):
            cp_kv[p][0].wait()
            cp_kv[p][1].wait()
        s1 = scores(*p1)
        s2 = scores(*p2)
        finish(*p1, s1)
        finish(*p2, s2)

    def wo_tile(slot, h, c):
        h0, k0 = _wo_loc(h, c, 0)
        h1, k1 = _wo_loc(h, c, 1)
        return jnp.concatenate([wo_all[slot, h0, k0], wo_all[slot, h1, k1]], axis=0)

    def outproj(jobs, first=False, rblk=SQ):
        for c, parts in jobs.items():
            tiles = [wo_tile(slot, h, c) for (slot, h) in parts]
            for r0 in range(0, ROWS, rblk):
                acc = None
                for (slot, h), w in zip(parts, tiles):
                    col0 = slot * 256 + h * 128
                    t = jnp.dot(ctx[r0:r0 + rblk, col0:col0 + 128], w,
                                preferred_element_type=F32)
                    acc = t if acc is None else acc + t
                b, rr = divmod(r0, SQ)
                if first:
                    out_ref[b, rr:rr + rblk, c * 128:(c + 1) * 128] = acc
                else:
                    out_ref[b, rr:rr + rblk, c * 128:(c + 1) * 128] += acc

    attend2((0, 0), (0, 1))

    recv_wait(wq_all.at[1, 0], rq(1, 0))
    send(wq_all.at[1, 0], wq_all.at[3, 0], rq(3, 0), right)
    send(wo_all.at[0, 1], wo_all.at[1, 1], ro(1, 1), right)
    recv_wait(wq_all.at[2, 1], rq(2, 1))
    send(wq_all.at[2, 1], wq_all.at[3, 1], rq(3, 1), left)
    send(wo_all.at[0, 0], wo_all.at[2, 0], ro(2, 0), left)

    attend2((1, 0), (2, 1))
    outproj({c: [(0, 0), (0, 1)] for c in range(4)}, first=True)

    recv_wait(wqs.at[0], rf[0])
    recv_wait(wqs.at[1], rf[1])
    recv_wait(wq_all.at[1, 1, rest], rq(1, 1))
    recv_wait(wq_all.at[2, 0, rest], rq(2, 0))
    wq_all[1, 1, 0:NF, :] = wqs[0].astype(BF)
    wq_all[2, 0, 0:NF, :] = wqs[1].astype(BF)
    attend2((1, 1), (2, 0))

    recv_wait(wo_all.at[1, 0], ro(1, 0))
    for i, (k0, n) in enumerate(WO_FWD):
        send(wo_all.at[1, 0, pl.ds(k0, n)], wo_all.at[3, 0, pl.ds(k0, n)],
             rod(0, i), right)
    recv_wait(wo_all.at[2, 1], ro(2, 1))
    for i, (k0, n) in enumerate(WO_FWD):
        send(wo_all.at[2, 1, pl.ds(k0, n)], wo_all.at[3, 1, pl.ds(k0, n)],
             rod(1, i), left)
    outproj({c: [(1, 0), (2, 1)] for c in range(3)})

    recv_wait(wq_all.at[3, 0], rq(3, 0))
    recv_wait(wq_all.at[3, 1], rq(3, 1))
    attend2((3, 0), (3, 1))

    pl.when(early_r)(fr.wait_send)
    pl.when(early_l)(fl.wait_send)
    pl.when(jnp.logical_not(early_r))(gr.wait_send)
    pl.when(jnp.logical_not(early_l))(gl.wait_send)

    recv_wait(wo_all.at[1, 1], ro(1, 1))
    recv_wait(wo_all.at[2, 0], ro(2, 0))
    jobs = {c: [(1, 1), (2, 0)] for c in range(3)}
    jobs[3] = [(1, 0), (1, 1), (2, 0), (2, 1)]
    outproj(jobs)

    for i, (k0, n) in enumerate(WO_FWD):
        recv_wait(wo_all.at[3, 0, pl.ds(k0, n)], rod(0, i))
        recv_wait(wo_all.at[3, 1, pl.ds(k0, n)], rod(1, i))
        if i < 3:
            outproj({i: [(3, 0), (3, 1)]})
        else:
            outproj({3: [(3, i - 3)]}, rblk=128)

    for s in sends:
        s.wait_send()


def pallas_dist_sparse_attn_blocksparse_qseq_b2_sq256_skv256_hq4_dh64_kernel(
    x: jax.Array,
    Wq: jax.Array,
    K_ext: jax.Array,
    V_ext: jax.Array,
    Wo: jax.Array,
):
    kt = jnp.transpose(K_ext, (0, 2, 3, 1)).reshape(B, 8, 128, SKV)
    vt = jnp.transpose(V_ext, (0, 2, 3, 1)).reshape(B, 8, 128, SKV)

    params = dict(collective_id=0, vmem_limit_bytes=64 * 1024 * 1024)
    if hasattr(pltpu.CompilerParams, "disable_semaphore_checks"):
        params["disable_semaphore_checks"] = True

    hbm = pl.BlockSpec(memory_space=pltpu.MemorySpace.HBM)
    return pl.pallas_call(
        _kernel,
        out_shape=jax.ShapeDtypeStruct((B, SQ, DM), F32),
        in_specs=[hbm] * 5,
        out_specs=pl.BlockSpec(memory_space=pltpu.VMEM),
        scratch_shapes=[
            pltpu.VMEM((B, SQ, DM), F32),
            pltpu.VMEM((ROWS, DM), BF),
            pltpu.VMEM((DM, 256), F32),
            pltpu.VMEM((256, DM), F32),
            pltpu.VMEM((4, 2, DM, 128), BF),
            pltpu.VMEM((4, 2, 8, DH, 128), BF),
            pltpu.VMEM((4, 2, B, 128, SKV), F32),
            pltpu.VMEM((4, 2, B, 128, SKV), F32),
            pltpu.VMEM((ROWS, 1024), BF),
            pltpu.VMEM((2, NF, 128), F32),
            pltpu.SemaphoreType.DMA((24,)),
            pltpu.SemaphoreType.DMA((1,)),
            pltpu.SemaphoreType.DMA((22,)),
            pltpu.SemaphoreType.REGULAR,
        ],
        compiler_params=pltpu.CompilerParams(**params),
    )(x, Wq, kt, vt, Wo)
```

```python
import jax
import jax.numpy as jnp
from jax import lax
from jax.experimental import pallas as pl
from jax.experimental.pallas import tpu as pltpu

N_DEV = 4
B = 2
SQ = 256
SKV = 256
DM = 512
DH = 64
BLK = 64
ROWS = B * SQ
NEG = -1e9
BF = jnp.bfloat16
F32 = jnp.float32
NT = (((1,), (1,)), ((), ()))
MESH = pl.DeviceIdType.MESH

SLOT_OFF = (0, 3, 1, 2)
WQ_PIECES = ((0, 16), (16, 48), (64, 64), (128, 128), (256, 256))
NF = 32
PAIR_ORDER = ((0, 0), (0, 1), (1, 0), (2, 1), (1, 1), (2, 0), (3, 0), (3, 1))
WO_FWD = ((0, 2), (2, 2), (4, 2), (6, 1), (7, 1))


def _wo_loc(h, c, a):
    if c < 3:
        return h, 2 * c + a
    return a, 6 + h


def _kernel(x_hbm, wq_hbm, kt_hbm, vt_hbm, wo_hbm, out_ref,
            xf, xb, wqf, wof, wq_all, wo_all, ktf, vtf, ctx, wqs,
            lsem, ssem, rsem, ready):
    me = lax.axis_index("i")
    left = (me + 3) & 3
    right = (me + 1) & 3
    odd = (me & 1) == 1

    cp_wq = [
        pltpu.make_async_copy(wq_hbm.at[pl.ds(r0, n)], wqf.at[pl.ds(r0, n)],
                              lsem.at[i])
        for i, (r0, n) in enumerate(WQ_PIECES)
    ]
    cp_wq[0].start()

    bar = pltpu.get_barrier_semaphore()

    @pl.when(me != 2)
    def _():
        for nbr in (left, right):
            pl.semaphore_signal(bar, inc=1, device_id=(nbr,), device_id_type=MESH)

    @pl.when(me == 2)
    def _():
        pl.semaphore_wait(bar, 2)
        for nbr in (left, right):
            pl.semaphore_signal(ready, inc=1, device_id=(nbr,), device_id_type=MESH)

    @pl.when(odd)
    def _():
        pl.semaphore_wait(bar, 1)

    sends = []

    def rcopy(src, dst, ridx, tgt):
        return pltpu.make_async_remote_copy(
            src, dst, ssem.at[0], rsem.at[ridx],
            device_id=(tgt,), device_id_type=MESH)

    def send(src, dst, ridx, tgt):
        c = rcopy(src, dst, ridx, tgt)
        c.start()
        sends.append(c)

    def recv_wait(dst, ridx):
        rcopy(dst, dst, ridx, me).wait_recv()

    def rq(slot, h):
        return (slot - 1) * 2 + h

    def ro(slot, half):
        return 6 + (slot - 1) * 2 + half

    def rod(half, k):
        return 10 + half * 5 + k

    rf = (20, 21)

    top = pl.ds(0, NF)
    fr = rcopy(wq_hbm.at[top, pl.ds(128, 128)], wqs.at[0], rf[0], right)
    fl = rcopy(wq_hbm.at[top, pl.ds(0, 128)], wqs.at[1], rf[1], left)
    early_r = me >= 2
    early_l = (me == 1) | (me == 2)
    pl.when(early_r)(fr.start)
    pl.when(early_l)(fl.start)
    gr = rcopy(wqf.at[top, pl.ds(128, 128)], wqs.at[0], rf[0], right)
    gl = rcopy(wqf.at[top, pl.ds(0, 128)], wqs.at[1], rf[1], left)

    for c in cp_wq[1:]:
        c.start()
    cp_wo = pltpu.make_async_copy(wo_hbm, wof, lsem.at[7])
    cp_wo.start()
    cp_x = []
    for b in range(B):
        c = pltpu.make_async_copy(x_hbm.at[b], xf.at[b], lsem.at[5 + b])
        c.start()
        cp_x.append(c)
    cp_kv = {}
    for i, (s, h) in enumerate(PAIR_ORDER):
        pr = 2 * ((me + SLOT_OFF[s]) & 3) + h
        ck = pltpu.make_async_copy(kt_hbm.at[:, pr], ktf.at[s, h],
                                   lsem.at[8 + 2 * i])
        cv = pltpu.make_async_copy(vt_hbm.at[:, pr], vtf.at[s, h],
                                   lsem.at[9 + 2 * i])
        ck.start()
        cv.start()
        cp_kv[(s, h)] = (ck, cv)

    to_r, to_l = [], []
    for i, (r0, n) in enumerate(WQ_PIECES):
        cp_wq[i].wait()
        for h in range(2):
            wq_all[0, h, r0:r0 + n, :] = (
                wqf[r0:r0 + n, h * 128:(h + 1) * 128].astype(BF))
        if i == 0:
            @pl.when(me == 0)
            def _():
                pl.semaphore_wait(bar, 2)
        rows = pl.ds(r0, n)
        cr = rcopy(wq_all.at[0, 0, rows], wq_all.at[1, 0, rows], rq(1, 0), right)
        cl = rcopy(wq_all.at[0, 1, rows], wq_all.at[2, 1, rows], rq(2, 1), left)
        to_r.append(cr)
        to_l.append(cl)
        pl.when(me != 1)(cr.start)
        pl.when(me != 3)(cl.start)
    sends += to_r + to_l

    @pl.when(odd)
    def _():
        pl.semaphore_wait(ready, 1)

    @pl.when(me == 1)
    def _():
        for c in to_r:
            c.start()

    @pl.when(me == 3)
    def _():
        for c in to_l:
            c.start()

    pl.when(jnp.logical_not(early_r))(gr.start)
    pl.when(jnp.logical_not(early_l))(gl.start)
    rest = pl.ds(NF, DM - NF)
    send(wq_all.at[0, 1, rest], wq_all.at[1, 1, rest], rq(1, 1), right)
    send(wq_all.at[0, 0, rest], wq_all.at[2, 0, rest], rq(2, 0), left)

    cp_wo.wait()
    for h in range(2):
        for c in range(4):
            for a in range(2):
                hf, k = _wo_loc(h, c, a)
                r0 = h * 128 + a * DH
                wo_all[0, hf, k] = wof[r0:r0 + DH, c * 128:(c + 1) * 128].astype(BF)
    send(wo_all.at[0, 0], wo_all.at[1, 0], ro(1, 0), right)
    send(wo_all.at[0, 1], wo_all.at[2, 1], ro(2, 1), left)

    for b in range(B):
        cp_x[b].wait()
        xb[b * SQ:(b + 1) * SQ, :] = xf[b].astype(BF)

    row = lax.broadcasted_iota(jnp.int32, (2 * BLK, SKV), 0)
    col = lax.broadcasted_iota(jnp.int32, (2 * BLK, SKV), 1)
    qb = me * (SQ // BLK) + 1 + row // BLK
    kb = col // BLK
    mask_mid = (qb == kb) | (kb == 0) | (lax.rem(qb + kb, 3) == 0)
    xk = 3 - lax.rem(me, 3)
    col1 = lax.broadcasted_iota(jnp.int32, (16, SKV), 1) // BLK
    off_ind = jnp.where((col1 == 0) | (col1 == xk), 0.0, 1.0).astype(BF)
    lo128 = lax.broadcasted_iota(jnp.int32, (128, 128), 1) < DH
    hi128 = jnp.logical_not(lo128)
    zero = jnp.zeros((128, 128), BF)
    ones_m = jnp.ones((DH, SKV), BF)
    ones_o = jnp.ones((DH, 128), BF)

    def gather_keys(t):
        t01 = t[:, :128]
        t23 = t[:, 128:]
        y = jnp.where(xk == 2, pltpu.roll(t23, 64, 1), t23)
        y = jnp.where(xk == 1, t01, y)
        return jnp.where(lo128, t01, y)

    def scores(slot, h):
        q = jnp.dot(xb[...], wq_all[slot, h], preferred_element_type=F32)
        q = (q * 0.125).astype(BF)
        out = []
        for b in range(B):
            ktf32 = ktf[slot, h, b]
            kt = ktf32.astype(BF)
            kg = gather_keys(ktf32).astype(BF)
            r0 = b * SQ
            qm = q[r0 + 64:r0 + 192]
            qo = jnp.concatenate([q[r0:r0 + 64], q[r0 + 192:r0 + 256]], axis=0)
            sm = [jnp.dot(jnp.where(sel, qm, zero), kt, preferred_element_type=F32)
                  for sel in (lo128, hi128)]
            so = [jnp.dot(jnp.where(sel, qo, zero), kg, preferred_element_type=F32)
                  for sel in (lo128, hi128)]
            out.append((sm, so))
        return out

    def finish(slot, h, sc_all):
        col0 = slot * 256 + h * 128
        for b in range(B):
            sm, so = sc_all[b]
            vtf32 = vtf[slot, h, b]
            vt = vtf32.astype(BF)
            vg = gather_keys(vtf32).astype(BF)
            vts = (jnp.concatenate([vt[:DH], ones_m], axis=0),
                   jnp.concatenate([ones_m, vt[DH:]], axis=0))
            vgs = (jnp.concatenate([vg[:DH], ones_o], axis=0),
                   jnp.concatenate([ones_o, vg[DH:]], axis=0))
            r0 = b * SQ
            rm, rout = [], []
            for a in range(2):
                s = jnp.where(mask_mid, sm[a], NEG)
                m = jnp.max(s, axis=-1, keepdims=True)
                p = jnp.exp(s - m).astype(BF)
                lhs = jnp.concatenate([p, off_ind], axis=0)
                rm.append(lax.dot_general(lhs, vts[a], NT,
                                          preferred_element_type=F32))
            for a in range(2):
                s = so[a]
                m = jnp.maximum(jnp.max(s, axis=-1, keepdims=True), NEG)
                p = jnp.exp(s - m).astype(BF)
                r = lax.dot_general(p, vgs[a], NT, preferred_element_type=F32)
                rout.append(r + jnp.exp(NEG - m) * rm[a][128:129])
            num = jnp.where(lo128, rm[0][:128], rm[1][:128])
            den = pltpu.roll(jnp.where(lo128, rm[1][:128], rm[0][:128]), 64, 1)
            ctx[r0 + 64:r0 + 192, col0:col0 + 128] = (num / den).astype(BF)
            num = jnp.where(lo128, rout[0], rout[1])
            den = pltpu.roll(jnp.where(lo128, rout[1], rout[0]), 64, 1)
            c = (num / den).astype(BF)
            ctx[r0:r0 + 64, col0:col0 + 128] = c[:64]
            ctx[r0 + 192:r0 + 256, col0:col0 + 128] = c[64:]

    def attend2(p1, p2):
        for p in (p1, p2):
            cp_kv[p][0].wait()
            cp_kv[p][1].wait()
        s1 = scores(*p1)
        s2 = scores(*p2)
        finish(*p1, s1)
        finish(*p2, s2)

    def wo_tile(slot, h, c):
        h0, k0 = _wo_loc(h, c, 0)
        h1, k1 = _wo_loc(h, c, 1)
        return jnp.concatenate([wo_all[slot, h0, k0], wo_all[slot, h1, k1]], axis=0)

    def outproj(jobs, first=False, rblk=SQ):
        for c, parts in jobs.items():
            tiles = [wo_tile(slot, h, c) for (slot, h) in parts]
            for r0 in range(0, ROWS, rblk):
                acc = None
                for (slot, h), w in zip(parts, tiles):
                    col0 = slot * 256 + h * 128
                    t = jnp.dot(ctx[r0:r0 + rblk, col0:col0 + 128], w,
                                preferred_element_type=F32)
                    acc = t if acc is None else acc + t
                b, rr = divmod(r0, SQ)
                if first:
                    out_ref[b, rr:rr + rblk, c * 128:(c + 1) * 128] = acc
                else:
                    out_ref[b, rr:rr + rblk, c * 128:(c + 1) * 128] += acc

    attend2((0, 0), (0, 1))

    recv_wait(wq_all.at[1, 0], rq(1, 0))
    send(wq_all.at[1, 0], wq_all.at[3, 0], rq(3, 0), right)
    send(wo_all.at[0, 1], wo_all.at[1, 1], ro(1, 1), right)
    recv_wait(wq_all.at[2, 1], rq(2, 1))
    send(wq_all.at[2, 1], wq_all.at[3, 1], rq(3, 1), left)
    send(wo_all.at[0, 0], wo_all.at[2, 0], ro(2, 0), left)

    attend2((1, 0), (2, 1))
    outproj({c: [(0, 0), (0, 1)] for c in range(4)}, first=True)

    recv_wait(wqs.at[0], rf[0])
    recv_wait(wqs.at[1], rf[1])
    recv_wait(wq_all.at[1, 1, rest], rq(1, 1))
    recv_wait(wq_all.at[2, 0, rest], rq(2, 0))
    wq_all[1, 1, 0:NF, :] = wqs[0].astype(BF)
    wq_all[2, 0, 0:NF, :] = wqs[1].astype(BF)
    attend2((1, 1), (2, 0))

    recv_wait(wo_all.at[1, 0], ro(1, 0))
    for i, (k0, n) in enumerate(WO_FWD):
        send(wo_all.at[1, 0, pl.ds(k0, n)], wo_all.at[3, 0, pl.ds(k0, n)],
             rod(0, i), right)
    recv_wait(wo_all.at[2, 1], ro(2, 1))
    for i, (k0, n) in enumerate(WO_FWD):
        send(wo_all.at[2, 1, pl.ds(k0, n)], wo_all.at[3, 1, pl.ds(k0, n)],
             rod(1, i), left)
    outproj({c: [(1, 0), (2, 1)] for c in range(3)})

    recv_wait(wq_all.at[3, 0], rq(3, 0))
    recv_wait(wq_all.at[3, 1], rq(3, 1))
    attend2((3, 0), (3, 1))

    pl.when(early_r)(fr.wait_send)
    pl.when(early_l)(fl.wait_send)
    pl.when(jnp.logical_not(early_r))(gr.wait_send)
    pl.when(jnp.logical_not(early_l))(gl.wait_send)

    recv_wait(wo_all.at[1, 1], ro(1, 1))
    recv_wait(wo_all.at[2, 0], ro(2, 0))
    jobs = {c: [(1, 1), (2, 0)] for c in range(3)}
    jobs[3] = [(1, 0), (1, 1), (2, 0), (2, 1)]
    outproj(jobs)

    for i, (k0, n) in enumerate(WO_FWD):
        recv_wait(wo_all.at[3, 0, pl.ds(k0, n)], rod(0, i))
        recv_wait(wo_all.at[3, 1, pl.ds(k0, n)], rod(1, i))
        if i < 3:
            outproj({i: [(3, 0), (3, 1)]})
        else:
            outproj({3: [(3, i - 3)]}, rblk=128)

    for s in sends:
        s.wait_send()


def pallas_dist_sparse_attn_blocksparse_qseq_b2_sq256_skv256_hq4_dh64_kernel(
    x: jax.Array,
    Wq: jax.Array,
    K_ext: jax.Array,
    V_ext: jax.Array,
    Wo: jax.Array,
):
    kt = jnp.transpose(K_ext, (0, 2, 3, 1)).reshape(B, 8, 128, SKV)
    vt = jnp.transpose(V_ext, (0, 2, 3, 1)).reshape(B, 8, 128, SKV)

    params = dict(collective_id=0, vmem_limit_bytes=64 * 1024 * 1024)
    if hasattr(pltpu.CompilerParams, "disable_semaphore_checks"):
        params["disable_semaphore_checks"] = True

    hbm = pl.BlockSpec(memory_space=pltpu.MemorySpace.HBM)
    return pl.pallas_call(
        _kernel,
        out_shape=jax.ShapeDtypeStruct((B, SQ, DM), F32),
        in_specs=[hbm] * 5,
        out_specs=pl.BlockSpec(memory_space=pltpu.VMEM),
        scratch_shapes=[
            pltpu.VMEM((B, SQ, DM), F32),
            pltpu.VMEM((ROWS, DM), BF),
            pltpu.VMEM((DM, 256), F32),
            pltpu.VMEM((256, DM), F32),
            pltpu.VMEM((4, 2, DM, 128), BF),
            pltpu.VMEM((4, 2, 8, DH, 128), BF),
            pltpu.VMEM((4, 2, B, 128, SKV), F32),
            pltpu.VMEM((4, 2, B, 128, SKV), F32),
            pltpu.VMEM((ROWS, 1024), BF),
            pltpu.VMEM((2, NF, 128), F32),
            pltpu.SemaphoreType.DMA((24,)),
            pltpu.SemaphoreType.DMA((1,)),
            pltpu.SemaphoreType.DMA((22,)),
            pltpu.SemaphoreType.REGULAR,
        ],
        compiler_params=pltpu.CompilerParams(**params),
    )(x, Wq, kt, vt, Wo)
```
